```python
import numpy as np

kernel_name = "dist_argmax_global_i_m8192_n1024"

def setup_inputs():
    return {"x": np.random.randn(32768, 1024).astype(np.float32)}

def reference(x: np.ndarray) -> np.ndarray:
    idx = np.argmax(x, axis=0).astype(np.float32)
    val = np.max(x, axis=0)
    return np.stack([val, idx], axis=0)
```

```python
import jax
import jax.numpy as jnp
from jax import lax
from jax.experimental import pallas as pl
from jax.experimental.pallas import tpu as pltpu

N_DEV = 4
K = 8
R = 8
D = 12


def _better(av, ai, bv, bi):
    a_nan = av != av
    b_nan = bv != bv
    gt = jnp.logical_and(jnp.logical_not(av <= bv), jnp.logical_not(b_nan))
    tie = jnp.logical_or(av == bv, jnp.logical_and(a_nan, b_nan))
    return jnp.logical_or(gt, jnp.logical_and(tie, ai < bi))


def pallas_dist_argmax_global_i_m8192_n1024_kernel(x: jax.Array):
    m, n = x.shape
    ns = D + 1
    sub = m // K
    ng = sub // R
    gs = sub // 8

    def body(x_hbm, out_ref, xbuf, msg, recv, obuf, copy_sems, tail_sems,
             send_sems, recv_sems, osem):
        me = lax.axis_index("i")

        def issue(t, slot, fine=False):
            for k in range(K):
                r0 = pl.multiple_of(k * sub + t * R, 8)
                sem = tail_sems.at[k] if fine else copy_sems.at[slot]
                pltpu.make_async_copy(
                    x_hbm.at[pl.ds(r0, R), :], xbuf.at[slot, pl.ds(k * R, R), :], sem
                ).start(priority=k % 2)

        def wait(slot):
            pltpu.make_async_copy(xbuf.at[slot], xbuf.at[slot], copy_sems.at[slot]).wait()

        def group(t, slot, v, g):
            gv = xbuf[slot, pl.ds(0, R), :]
            gg = jnp.zeros((8, n), jnp.int32)
            for k in range(1, K):
                xb = xbuf[slot, pl.ds(k * R, R), :]
                take = jnp.logical_and(jnp.logical_not(xb <= gv), gv == gv)
                gv = jnp.where(take, xb, gv)
                gg = jnp.where(take, k * gs, gg)
            gg = gg + t
            take = _better(gv, gg, v, g)
            return jnp.where(take, gv, v), jnp.where(take, gg, g)

        for t in range(D):
            issue(t, t % ns, fine=(t == ng - 1))
        barrier = pltpu.get_barrier_semaphore()
        for d in range(1, N_DEV):
            pl.semaphore_signal(barrier, inc=1, device_id=((me + d) % N_DEV,),
                                device_id_type=pl.DeviceIdType.MESH)

        v = jnp.full((8, n), -jnp.inf, jnp.float32)
        g = jnp.full((8, n), 2 ** 30, jnp.int32)

        n_main = ng - D - 1

        def step(t, carry):
            v, g = carry
            issue(t + D, (t + D) % ns)
            wait(t % ns)
            return group(t, t % ns, v, g)

        v, g = lax.fori_loop(0, n_main, step, (v, g))
        for t in range(n_main, ng):
            if t + D < ng:
                issue(t + D, (t + D) % ns, fine=(t + D == ng - 1))
            if t == ng - 1:
                pl.semaphore_wait(barrier, N_DEV - 1)
                slot = t % ns
                for k in range(K):
                    blk = xbuf.at[slot, pl.ds(k * R, R), :]
                    pltpu.make_async_copy(blk, blk, tail_sems.at[k]).wait()
                    xb = blk[...]
                    gk = jnp.full((8, n), k * gs + t, jnp.int32)
                    take = _better(xb, gk, v, g)
                    v = jnp.where(take, xb, v)
                    g = jnp.where(take, gk, g)
            else:
                wait(t % ns)
                v, g = group(t, t % ns, v, g)

        row = g * 8 + lax.broadcasted_iota(jnp.int32, (8, n), 0) + me * m
        rowf = row.astype(jnp.float32)
        for sh in (4, 2, 1):
            v2 = pltpu.roll(v, sh, 0)
            i2 = pltpu.roll(rowf, sh, 0)
            tk = _better(v2, i2, v, rowf)
            v = jnp.where(tk, v2, v)
            rowf = jnp.where(tk, i2, rowf)
        bv = v[0:1]
        bi = rowf[0:1]
        msg[0:1, :] = bv
        msg[1:2, :] = bi
        rdmas = {}
        for d in (2, 1, 3):
            r = pltpu.make_async_remote_copy(
                src_ref=msg, dst_ref=recv.at[d - 1], send_sem=send_sems.at[d - 1],
                recv_sem=recv_sems.at[d - 1],
                device_id=((me + d) % N_DEV,), device_id_type=pl.DeviceIdType.MESH)
            r.start()
            rdmas[d] = r
        for d in (1, 3, 2):
            rdmas[d].wait_recv()
            ov = recv[d - 1, 0:1, :]
            oi = recv[d - 1, 1:2, :]
            tk = _better(ov, oi, bv, bi)
            bv = jnp.where(tk, ov, bv)
            bi = jnp.where(tk, oi, bi)
        obuf[0:1, :] = bv
        obuf[1:2, :] = bi
        ocp = pltpu.make_async_copy(obuf, out_ref, osem)
        ocp.start()
        for r in rdmas.values():
            r.wait_send()
        ocp.wait()

    return pl.pallas_call(
        body,
        out_shape=jax.ShapeDtypeStruct((2, n), jnp.float32),
        in_specs=[pl.BlockSpec(memory_space=pl.ANY)],
        out_specs=pl.BlockSpec(memory_space=pl.ANY),
        scratch_shapes=[
            pltpu.VMEM((ns, K * R, n), jnp.float32),
            pltpu.VMEM((2, n), jnp.float32),
            pltpu.VMEM((N_DEV - 1, 2, n), jnp.float32),
            pltpu.VMEM((2, n), jnp.float32),
            pltpu.SemaphoreType.DMA((ns,)),
            pltpu.SemaphoreType.DMA((K,)),
            pltpu.SemaphoreType.DMA((N_DEV - 1,)),
            pltpu.SemaphoreType.DMA((N_DEV - 1,)),
            pltpu.SemaphoreType.DMA,
        ],
        compiler_params=pltpu.CompilerParams(
            collective_id=0,
            vmem_limit_bytes=64 * 1024 * 1024,
            disable_bounds_checks=True,
            disable_semaphore_checks=True,
        ),
    )(x)
```

```python
import jax
import jax.numpy as jnp
from jax import lax
from jax.experimental import pallas as pl
from jax.experimental.pallas import tpu as pltpu

N_DEV = 4
K = 8
R = 8
D = 12
UNITS = (8, 4, 2, 1, 1)
LANES = 128


def _merge(av, ai, bv, bi):
    a_lo = ai < bi
    keep_a = jnp.logical_or(bv <= av, av != av)
    keep_b = jnp.logical_or(av <= bv, bv != bv)
    v = jnp.where(a_lo, jnp.where(keep_a, av, bv), jnp.where(keep_b, bv, av))
    i = jnp.where(a_lo, jnp.where(keep_a, ai, bi), jnp.where(keep_b, bi, ai))
    return v, i


def _merge_lo_hi(lv, li, hv, hi):
    keep = jnp.logical_or(hv <= lv, lv != lv)
    return jnp.where(keep, lv, hv), jnp.where(keep, li, hi)


def _tournament(c, f):
    while len(c) > 1:
        nxt = [f(*c[i], *c[i + 1]) for i in range(0, len(c) - 1, 2)]
        if len(c) % 2:
            nxt.append(c[-1])
        c = nxt
    return c[0]


def pallas_dist_argmax_global_i_m8192_n1024_kernel(x: jax.Array):
    m, n = x.shape
    ns = D + 1
    nt = sum(UNITS)
    tg = nt // K
    sub = m // K
    nb = sub // R - tg
    gs = sub // 8
    ustart = [sum(UNITS[:u]) for u in range(len(UNITS))]
    unit_of = [u for u, cnt in enumerate(UNITS) for _ in range(cnt)]
    half = n // 2
    assert nt % K == 0 and m % (K * R) == 0 and n == 8 * LANES
    assert all(s // K == (s + cnt - 1) // K for s, cnt in zip(ustart, UNITS))
    assert N_DEV * m <= 1 << 16

    def body(x_hbm, out_ref, xbuf, tbuf, pre, msg, recv,
             copy_sems, tail_sems, send_sems, recv_sems):
        me = lax.axis_index("i")

        def issue(t, slot):
            for k in range(K):
                r0 = pl.multiple_of(k * sub + t * R, 8)
                pltpu.make_async_copy(
                    x_hbm.at[pl.ds(r0, R), :], xbuf.at[slot, pl.ds(k * R, R), :],
                    copy_sems.at[slot]).start(priority=k % 2)

        def issue_tail(j):
            for k in range(K):
                b = j * K + k
                pltpu.make_async_copy(
                    x_hbm.at[pl.ds(k * sub + (nb + j) * R, R), :],
                    tbuf.at[pl.ds(b * R, R), :],
                    tail_sems.at[unit_of[b]]).start(priority=k % 2)

        def proc(t, carry):
            v, g = carry
            slot = t % ns
            pltpu.make_async_copy(xbuf.at[slot], xbuf.at[slot], copy_sems.at[slot]).wait()
            gv = xbuf[slot, pl.ds(0, R), :]
            gg = jnp.zeros((8, n), jnp.int32)
            for k in range(1, K):
                xb = xbuf[slot, pl.ds(k * R, R), :]
                keep = jnp.logical_or(xb <= gv, gv != gv)
                gv = jnp.where(keep, gv, xb)
                gg = jnp.where(keep, gg, k * gs)
            return _merge(gv, gg + t, v, g)

        def step(t, carry):
            issue(t + D, (t + D) % ns)
            return proc(t, carry)

        for t in range(D):
            issue(t, t % ns)
        barrier = pltpu.get_barrier_semaphore()
        for d in range(1, N_DEV):
            pl.semaphore_signal(barrier, inc=1, device_id=((me + d) % N_DEV,),
                                device_id_type=pl.DeviceIdType.MESH)

        v = jnp.full((8, n), -jnp.inf, jnp.float32)
        g = jnp.full((8, n), 2 ** 26, jnp.int32)
        v, g = lax.fori_loop(0, nb - D, step, (v, g))
        for j in range(tg):
            issue_tail(j)
            v, g = proc(nb - D + j, (v, g))
        v, g = lax.fori_loop(nb - D + tg, nb, proc, (v, g))

        pl.semaphore_wait(barrier, N_DEV - 1)

        row = g * 8 + lax.broadcasted_iota(jnp.int32, (8, n), 0)
        pre[0:8, :] = v
        pre[8:16, :] = row.astype(jnp.float32)
        bv, bi = _tournament(
            [(pre[s:s + 1, :], pre[8 + s:9 + s, :]) for s in range(8)], _merge)

        for u, cnt in enumerate(UNITS):
            b0 = ustart[u]
            blk = tbuf.at[pl.ds(b0 * R, cnt * R), :]
            pltpu.make_async_copy(blk, blk, tail_sems.at[u]).wait()
            c = []
            for b in range(b0, b0 + cnt):
                j, k = divmod(b, K)
                r0 = k * sub + (nb + j) * R
                c += [(tbuf[b * R + s:b * R + s + 1, :],
                       jnp.full((1, n), float(r0 + s), jnp.float32)) for s in range(R)]
            tv, ti = _tournament(c, _merge_lo_hi)
            if b0 == nt - 1:
                bv, bi = _merge_lo_hi(bv, bi, tv, ti)
            else:
                bv, bi = _merge(tv, ti, bv, bi)

        bv = bv.reshape(8, LANES)
        gi = bi.reshape(8, LANES).astype(jnp.int32) + me * m
        packed = jnp.bitwise_or(gi[0:4], jnp.left_shift(gi[4:8], 16))
        msg[0:1, 0:n] = lax.bitcast_convert_type(bv, jnp.int32).reshape(1, n)
        msg[0:1, n:n + half] = packed.reshape(1, half)
        bi = gi.astype(jnp.float32)

        rdmas = {}
        for d in (2, 1, 3):
            rdmas[d] = pltpu.make_async_remote_copy(
                src_ref=msg, dst_ref=recv.at[d - 1],
                send_sem=send_sems.at[d - 1], recv_sem=recv_sems.at[d - 1],
                device_id=((me + d) % N_DEV,), device_id_type=pl.DeviceIdType.MESH)
            rdmas[d].start()
        for d in (1, 3, 2):
            if d == 2:
                for r in rdmas.values():
                    r.wait_send()
            rdmas[d].wait_recv()
            ov = lax.bitcast_convert_type(
                recv[d - 1, 0:1, 0:n].reshape(8, LANES), jnp.float32)
            w = recv[d - 1, 0:1, n:n + half].reshape(4, LANES)
            oi = jnp.concatenate(
                [jnp.bitwise_and(w, 0xFFFF), lax.shift_right_logical(w, 16)],
                axis=0).astype(jnp.float32)
            bv, bi = _merge(ov, oi, bv, bi)
        out_ref[0:1, :] = bv.reshape(1, n)
        out_ref[1:2, :] = bi.reshape(1, n)

    return pl.pallas_call(
        body,
        out_shape=jax.ShapeDtypeStruct((2, n), jnp.float32),
        in_specs=[pl.BlockSpec(memory_space=pl.ANY)],
        out_specs=pl.BlockSpec(memory_space=pltpu.VMEM),
        scratch_shapes=[
            pltpu.VMEM((ns, K * R, n), jnp.float32),
            pltpu.VMEM((nt * R, n), jnp.float32),
            pltpu.VMEM((16, n), jnp.float32),
            pltpu.VMEM((1, n + half), jnp.int32),
            pltpu.VMEM((N_DEV - 1, 1, n + half), jnp.int32),
            pltpu.SemaphoreType.DMA((ns,)),
            pltpu.SemaphoreType.DMA((len(UNITS),)),
            pltpu.SemaphoreType.DMA((N_DEV - 1,)),
            pltpu.SemaphoreType.DMA((N_DEV - 1,)),
        ],
        compiler_params=pltpu.CompilerParams(
            collective_id=0,
            vmem_limit_bytes=64 * 1024 * 1024,
            disable_bounds_checks=True,
            disable_semaphore_checks=True,
        ),
    )(x)
```

```python
import jax
import jax.numpy as jnp
from jax import lax
from jax.experimental import pallas as pl
from jax.experimental.pallas import tpu as pltpu

N_DEV = 4
K = 8
R = 8
D = 12
UNITS = (8, 4, 2, 1, 1)
LANES = 128


def _merge(av, ai, bv, bi):
    a_lo = ai < bi
    keep_a = jnp.logical_or(bv <= av, av != av)
    keep_b = jnp.logical_or(av <= bv, bv != bv)
    v = jnp.where(a_lo, jnp.where(keep_a, av, bv), jnp.where(keep_b, bv, av))
    i = jnp.where(a_lo, jnp.where(keep_a, ai, bi), jnp.where(keep_b, bi, ai))
    return v, i


def _merge_lo_hi(lv, li, hv, hi):
    keep = jnp.logical_or(hv <= lv, lv != lv)
    return jnp.where(keep, lv, hv), jnp.where(keep, li, hi)


def _tournament(c, f):
    while len(c) > 1:
        nxt = [f(*c[i], *c[i + 1]) for i in range(0, len(c) - 1, 2)]
        if len(c) % 2:
            nxt.append(c[-1])
        c = nxt
    return c[0]


def pallas_dist_argmax_global_i_m8192_n1024_kernel(x: jax.Array):
    m, n = x.shape
    ns = D + 1
    nt = sum(UNITS)
    tg = nt // K
    sub = m // K
    nb = sub // R - tg
    gs = sub // 8
    ustart = [sum(UNITS[:u]) for u in range(len(UNITS))]
    unit_of = [u for u, cnt in enumerate(UNITS) for _ in range(cnt)]
    half = n // 2
    assert nt % K == 0 and m % (K * R) == 0 and n == 8 * LANES
    assert all(s // K == (s + cnt - 1) // K for s, cnt in zip(ustart, UNITS))
    assert N_DEV * m <= 1 << 16

    def body(x_hbm, out_ref, xbuf, tbuf, pre_v, pre_i, msg, recv,
             copy_sems, tail_sems, send_sems, recv_sems):
        me = lax.axis_index("i")

        def issue(t, slot):
            for k in range(K):
                r0 = pl.multiple_of(k * sub + t * R, 8)
                pltpu.make_async_copy(
                    x_hbm.at[pl.ds(r0, R), :], xbuf.at[slot, pl.ds(k * R, R), :],
                    copy_sems.at[slot]).start(priority=k % 2)

        def issue_tail(j):
            for k in range(K):
                b = j * K + k
                pltpu.make_async_copy(
                    x_hbm.at[pl.ds(k * sub + (nb + j) * R, R), :],
                    tbuf.at[pl.ds(b * R, R), :],
                    tail_sems.at[unit_of[b]]).start(priority=k % 2)

        def proc(t, carry):
            v, g = carry
            slot = t % ns
            pltpu.make_async_copy(xbuf.at[slot], xbuf.at[slot], copy_sems.at[slot]).wait()
            gv = xbuf[slot, pl.ds(0, R), :]
            gg = jnp.zeros((8, n), jnp.int32)
            for k in range(1, K):
                xb = xbuf[slot, pl.ds(k * R, R), :]
                keep = jnp.logical_or(xb <= gv, gv != gv)
                gv = jnp.where(keep, gv, xb)
                gg = jnp.where(keep, gg, k * gs)
            return _merge(gv, gg + t, v, g)

        def step(t, carry):
            issue(t + D, (t + D) % ns)
            return proc(t, carry)

        for t in range(D):
            issue(t, t % ns)
        barrier = pltpu.get_barrier_semaphore()
        for d in range(1, N_DEV):
            pl.semaphore_signal(barrier, inc=1, device_id=((me + d) % N_DEV,),
                                device_id_type=pl.DeviceIdType.MESH)

        v = jnp.full((8, n), -jnp.inf, jnp.float32)
        g = jnp.full((8, n), 2 ** 26, jnp.int32)
        v, g = lax.fori_loop(0, nb - D, step, (v, g))
        for j in range(tg):
            issue_tail(j)
            v, g = proc(nb - D + j, (v, g))
        v, g = lax.fori_loop(nb - D + tg, nb, proc, (v, g))

        pl.semaphore_wait(barrier, N_DEV - 1)

        offset = me * m
        pre_v[...] = v
        pre_i[...] = g * 8 + lax.broadcasted_iota(jnp.int32, (8, n), 0) + offset
        bv, bi = _tournament(
            [(pre_v[s:s + 1, :], pre_i[s:s + 1, :]) for s in range(8)], _merge)

        base = jnp.full((1, n), offset, jnp.int32)
        for u, cnt in enumerate(UNITS):
            b0 = ustart[u]
            blk = tbuf.at[pl.ds(b0 * R, cnt * R), :]
            pltpu.make_async_copy(blk, blk, tail_sems.at[u]).wait()
            c = []
            for b in range(b0, b0 + cnt):
                j, k = divmod(b, K)
                r0 = k * sub + (nb + j) * R
                c += [(tbuf[b * R + s:b * R + s + 1, :], base + (r0 + s))
                      for s in range(R)]
            tv, ti = _tournament(c, _merge_lo_hi)
            if b0 == nt - 1:
                bv, bi = _merge_lo_hi(bv, bi, tv, ti)
            else:
                bv, bi = _merge(tv, ti, bv, bi)

        lo = lax.broadcasted_iota(jnp.int32, (8, LANES), 0) < 4
        bv = bv.reshape(8, LANES)
        bi = bi.reshape(8, LANES)
        bits = lax.bitcast_convert_type(bv, jnp.int32)
        packed = jnp.bitwise_or(pltpu.roll(bi, 4, 0), jnp.left_shift(bi, 16))
        msg[0:1, half:half + n] = bits.reshape(1, n)
        msg[0:1, 0:n] = jnp.where(lo, bits, packed).reshape(1, n)

        rdmas = {}
        for d in (2, 1, 3):
            rdmas[d] = pltpu.make_async_remote_copy(
                src_ref=msg, dst_ref=recv.at[d - 1],
                send_sem=send_sems.at[d - 1], recv_sem=recv_sems.at[d - 1],
                device_id=((me + d) % N_DEV,), device_id_type=pl.DeviceIdType.MESH)
            rdmas[d].start()
        for d in (1, 3, 2):
            if d == 2:
                for r in rdmas.values():
                    r.wait_send()
            rdmas[d].wait_recv()
            hi_rows = recv[d - 1, 0:1, half:half + n].reshape(8, LANES)
            lo_rows = recv[d - 1, 0:1, 0:n].reshape(8, LANES)
            ov = lax.bitcast_convert_type(jnp.where(lo, lo_rows, hi_rows), jnp.float32)
            oi = jnp.where(lo, jnp.bitwise_and(hi_rows, 0xFFFF),
                           lax.shift_right_logical(lo_rows, 16))
            bv, bi = _merge(ov, oi, bv, bi)
        out_ref[0:1, :] = bv.reshape(1, n)
        out_ref[1:2, :] = bi.astype(jnp.float32).reshape(1, n)

    return pl.pallas_call(
        body,
        out_shape=jax.ShapeDtypeStruct((2, n), jnp.float32),
        in_specs=[pl.BlockSpec(memory_space=pl.ANY)],
        out_specs=pl.BlockSpec(memory_space=pltpu.VMEM),
        scratch_shapes=[
            pltpu.VMEM((ns, K * R, n), jnp.float32),
            pltpu.VMEM((nt * R, n), jnp.float32),
            pltpu.VMEM((8, n), jnp.float32),
            pltpu.VMEM((8, n), jnp.int32),
            pltpu.VMEM((1, n + half), jnp.int32),
            pltpu.VMEM((N_DEV - 1, 1, n + half), jnp.int32),
            pltpu.SemaphoreType.DMA((ns,)),
            pltpu.SemaphoreType.DMA((len(UNITS),)),
            pltpu.SemaphoreType.DMA((N_DEV - 1,)),
            pltpu.SemaphoreType.DMA((N_DEV - 1,)),
        ],
        compiler_params=pltpu.CompilerParams(
            collective_id=0,
            vmem_limit_bytes=64 * 1024 * 1024,
            disable_bounds_checks=True,
            disable_semaphore_checks=True,
        ),
    )(x)
```
